```python
import numpy as np

kernel_name = "dist_moe_top2_ep_n2048_d512_e4_h1024"

def setup_inputs():
    x = np.random.randn(2048, 512).astype(np.float32)
    router_W = np.random.randn(512, 16).astype(np.float32) * 0.1
    scores64 = x.astype(np.float64) @ router_W.astype(np.float64)
    route_idx = np.argsort(-scores64, axis=-1)[:, :2].astype(np.int32)
    expert_W = np.random.randn(16, 512, 1024).astype(np.float32) * 0.02
    return {"x": x, "router_W": router_W, "route_idx": route_idx, "expert_W": expert_W}

def reference(x, router_W, route_idx, expert_W):
    scores = x @ router_W
    s_max = scores.max(axis=-1, keepdims=True)
    probs = np.exp(scores - s_max)
    probs = probs / probs.sum(axis=-1, keepdims=True)
    out = np.zeros((2048, 1024), dtype=np.float32)
    for i in range(2048):
        e0, e1 = int(route_idx[i, 0]), int(route_idx[i, 1])
        g0, g1 = probs[i, e0], probs[i, e1]
        gs = g0 + g1
        out[i] = (g0 / gs) * (x[i] @ expert_W[e0]) + (g1 / gs) * (x[i] @ expert_W[e1])
    return out
```

```python
import jax
import jax.numpy as jnp
from jax import lax
from jax.experimental import pallas as pl
from jax.experimental.pallas import tpu as pltpu

I32 = jnp.int32
U32 = jnp.uint32
F32 = jnp.float32
BF16 = jnp.bfloat16
MESH = pl.DeviceIdType.MESH

N, D, H = 2048, 512, 1024
NDEV, EPC = 4, 4
NW, T, CAP = 16, 128, 32
BM = 288
XC = 8
XT = N // XC
GU = 16
LA = 2
RMAX = 2 * N + BM
TRASH = RMAX


def _iota(shape, dim):
    return lax.broadcasted_iota(I32, shape, dim)


def _cum_tot(masks, uj):
    r = masks[0].shape[0]
    h = jnp.concatenate([jnp.where(m, 1.0, 0.0).astype(BF16) for m in masks], axis=0)
    ct = jnp.dot(h, uj, preferred_element_type=F32)
    cum = [ct[r * i:r * (i + 1), 0:128] for i in range(len(masks))]
    tot = [ct[r * i:r * (i + 1), 128:256] for i in range(len(masks))]
    return cum, tot


def _shift_left_flat(x, s):
    r = x.shape[0]
    row = _iota(x.shape, 0)
    lane = _iota(x.shape, 1)
    if s < 128:
        a = pltpu.roll(x, 128 - s, 1)
        b = pltpu.roll(a, r - 1, 0)
        y = jnp.where(lane < 128 - s, a, b)
        return jnp.where((lane >= 128 - s) & (row == r - 1), 0, y)
    rs = s // 128
    y = pltpu.roll(x, r - rs, 0)
    return jnp.where(row >= r - rs, 0, y)


def _shift_left_rows(x, s):
    lane = _iota(x.shape, 1)
    return jnp.where(lane < 128 - s, pltpu.roll(x, 128 - s, 1), 0)


def _compact(word, nbits, shift):
    for s in range(nbits):
        inc = shift(word, 1 << s)
        take = ((inc >> nbits) & (inc >> s) & 1) == 1
        stay = (((word >> nbits) & 1) == 1) & (((word >> s) & 1) == 0)
        word = jnp.where(take, inc, jnp.where(stay, word, 0))
    return word


def _routing_metadata(me, idx_v, dup_v, la_v, lb_v, gp_v, misc_v):
    ui = _iota((128, 256), 0)
    ul = _iota((128, 256), 1)
    uj = jnp.where((ui < ul) | (ul >= 128), 1.0, 0.0).astype(BF16)

    e0 = idx_v[pl.ds(0, NW, stride=2), :]
    e1 = idx_v[pl.ds(1, NW, stride=2), :]
    lane = _iota((NW, T), 1)
    c0 = e0 >> 2
    c1 = e1 >> 2
    dc = (c1 - c0) & 3
    pref = jnp.where(dc == 0, c0, jnp.where(dc == 2, NDEV, jnp.where((lane & 1) == 1, c0, c1)))
    masks = [pref == k for k in range(NDEV)]
    cum, tot = _cum_tot(masks, uj)
    rank = sum(jnp.where(masks[k], cum[k], 0.0) for k in range(NDEV))
    keep = (pref < NDEV) & (rank < CAP)
    (f,), _ = _cum_tot([jnp.logical_not(keep)], uj)
    free = [CAP - jnp.minimum(tot[k], float(CAP)) for k in range(NDEV)]
    p1 = free[0]
    p2 = p1 + free[1]
    p3 = p2 + free[2]
    spill = (f >= p1).astype(I32) + (f >= p2).astype(I32) + (f >= p3).astype(I32)
    owner = jnp.where(keep, pref, spill)
    omasks = [owner == k for k in range(NDEV)]
    qcum, _ = _cum_tot(omasks, uj)
    q = sum(jnp.where(omasks[k], qcum[k], 0.0) for k in range(NDEV)).astype(I32)
    gp_v[...] = (_iota((NW, T), 0) * T + owner * CAP + q) * 4

    dup_v[pl.ds(0, NW, stride=2), :] = owner
    dup_v[pl.ds(1, NW, stride=2), :] = owner
    oa = dup_v[...]
    ea = idx_v[...]
    local = (ea >> 2) == me
    cs = jnp.where(local, (ea & 3) * 4 + oa, -1)
    co = jnp.where(oa == me, ea, -1)
    cx = jnp.where(ea < EPC * me, oa, -1)
    ms = [cs == c for c in range(16)]
    mo = [co == c for c in range(16)]
    mx = [cx == k for k in range(NDEV)]
    cum_s, tot_s = _cum_tot(ms + [local], uj)
    cum_o, tot_o = _cum_tot(mo, uj)
    _, tot_x = _cum_tot(mx, uj)
    tri = jnp.where(_iota((40, 32), 1) < _iota((40, 32), 0), 1.0, 0.0).astype(BF16)
    tt = jnp.concatenate(tot_s + tot_o + tot_x, axis=1).astype(BF16)
    car = jnp.dot(tri, tt, preferred_element_type=F32)

    def blk(i):
        return car[:, 128 * i:128 * (i + 1)]

    lane1 = _iota((1, 128), 1)
    zrow = jnp.zeros((1, 128), I32)
    row_n, row_na, row_x, row_c = zrow, zrow, zrow, zrow
    base = jnp.zeros((1, 128), F32)
    r = jnp.zeros((32, 128), F32)
    for c in range(16):
        cb = blk(c)
        r = r + jnp.where(ms[c], cum_s[c] + cb[0:32] + base, 0.0)
        row_n = jnp.where(lane1 == c, cb[32:33].astype(I32), row_n)
        row_na = jnp.where(lane1 == c, cb[16:17].astype(I32), row_na)
        base = base + cb[32:33]
    locb = blk(16)
    rl = cum_s[16] + locb[0:32]
    base = jnp.zeros((1, 128), F32)
    sg = jnp.zeros((32, 128), F32)
    for c in range(16):
        cb = blk(17 + c)
        sg = sg + jnp.where(mo[c], cum_o[c] + cb[0:32] + base, 0.0)
        base = base + cb[32:33]
    for k in range(NDEV):
        row_x = jnp.where(lane1 == k, blk(33 + k)[32:33].astype(I32), row_x)
    rpc = 32 // XC
    for c in range(XC):
        row_c = jnp.where(lane1 == c, locb[rpc * (c + 1):rpc * (c + 1) + 1].astype(I32), row_c)
    misc_v[0:1, :] = row_n
    misc_v[1:2, :] = row_na
    misc_v[2:3, :] = row_x
    misc_v[3:4, :] = row_c
    misc_v[4:8, :] = jnp.zeros((4, 128), I32)

    aidx = _iota((32, 128), 0) * 128 + _iota((32, 128), 1)
    wa = jnp.where(local, (r.astype(I32) << 13) | (1 << 12) | (aidx - rl.astype(I32)), 0)
    wa = _compact(wa, 12, _shift_left_flat)
    a = aidx + (wa & 4095)
    tok = ((a >> 8) << 7) | (a & 127)
    la_v[...] = jnp.where(((wa >> 12) & 1) == 1, (tok * 4) | (((wa >> 13) * 4) << 16),
                          (TRASH * 4) << 16)

    dup_v[...] = sg.astype(I32)
    s0 = dup_v[pl.ds(0, NW, stride=2), :]
    s1 = dup_v[pl.ds(1, NW, stride=2), :]
    wb = jnp.where(owner == me, (s1 << 18) | (s0 << 8) | (1 << 7) | (lane - q), 0)
    wb = _compact(wb, 7, _shift_left_rows)
    tl = lane + (wb & 127)
    lb_v[...] = jnp.where(lane < CAP,
                          ((wb >> 8) & 1023) | (((wb >> 18) & 1023) << 10) | (tl << 20), 0)


def _unpack(p, i):
    return pltpu.unpack_elementwise(p, index=i, packed_dtype=BF16, unpacked_dtype=F32)


def _pack(lo, hi):
    return pltpu.pack_elementwise([lo, hi], packed_dtype=BF16)


def _body(x_hbm, rw_hbm, idx_hbm, w_hbm, out_hbm,
          idx_v, dup_v, rw_v, xs, xt, wv, lhs_t, lhs_b, yt, stg, gb, tmp, ost,
          la_v, lb_v, gp_v, misc_v, g0_v, g1_v,
          la_s, lb_s, gp_s, misc_s, g0_s, g1_s,
          lsem, xsem, wsem, osem, p1_send, p1_recv, p2_send, dl_recv, dr_recv, f_recv):
    me = lax.axis_index("i")
    right = (me + 1) % NDEV
    left = (me + NDEV - 1) % NDEV
    diag = (me + 2) % NDEV

    barrier = pltpu.get_barrier_semaphore()
    for peer in (right, left, diag):
        pl.semaphore_signal(barrier, inc=1, device_id=(peer,), device_id_type=MESH)

    idx_cp = pltpu.make_async_copy(idx_hbm, idx_v, lsem.at[0])
    rw_cp = pltpu.make_async_copy(rw_hbm, rw_v, lsem.at[1])
    idx_cp.start()

    def x_copy(c):
        rows = pl.ds(pl.multiple_of(c * XT, XT), XT)
        return pltpu.make_async_copy(x_hbm.at[rows], xs.at[rows], xsem.at[c])

    def w_copy(e, h):
        return pltpu.make_async_copy(w_hbm.at[e, :, pl.ds(512 * h, 512)], wv.at[2 * e + h],
                                     wsem.at[2 * e + h])

    for c in range(XC):
        x_copy(c).start()
    rw_cp.start()
    for e in range(EPC):
        for h in range(2):
            w_copy(e, h).start(priority=1)

    idx_cp.wait()
    _routing_metadata(me, idx_v, dup_v, la_v, lb_v, gp_v, misc_v)
    la_cp = pltpu.make_async_copy(la_v, la_s, lsem.at[2])
    misc_cp = pltpu.make_async_copy(misc_v, misc_s, lsem.at[3])
    lb_cp = pltpu.make_async_copy(lb_v, lb_s, lsem.at[4])
    gp_cp = pltpu.make_async_copy(gp_v, gp_s, lsem.at[5])
    for cp in (misc_cp, la_cp, lb_cp, gp_cp):
        cp.start()

    def relayout(c):
        x_copy(c).wait()
        rows = pl.ds(pl.multiple_of(c * XT, XT), XT)
        for j in range(4):
            xt[pl.ds(c * (XT * 4) + j, XT, stride=4), :] = xs[rows, 128 * j:128 * (j + 1)]

    npre = 2
    for c in range(npre):
        relayout(c)
    misc_cp.wait()
    la_cp.wait()

    def gather_group(g, carry):
        row = g >> 3
        l0 = (g & 7) * GU
        for u in range(GU):
            w = la_s[row, l0 + u]
            lhs_t[pl.ds(w >> 16, 4), :] = xt[pl.ds(w & 0xFFFF, 4), :]
        return carry

    def x_step(c, g0):
        @pl.when(c >= npre)
        def _():
            relayout(c)
        n = misc_s[3, c]
        g1 = jnp.where(c == XC - 1, (n + GU - 1) // GU, n // GU)
        lax.fori_loop(g0, g1, gather_group, 0)
        return g1

    lax.fori_loop(0, XC, x_step, 0)
    rw_cp.wait()

    def send_rows(src, dst, n, dev, grp):
        for bit in range(9, -1, -1):
            @pl.when(((n >> bit) & 1) == 1)
            def _():
                off = (n >> (bit + 1)) << (bit + 1)
                size = 4 << bit
                pltpu.make_async_remote_copy(
                    src_ref=yt.at[pl.ds((src + off) * 4, size)],
                    dst_ref=stg.at[pl.ds((dst + off) * 4, size)],
                    send_sem=p1_send, recv_sem=p1_recv.at[grp],
                    device_id=(dev,), device_id_type=MESH).start()

    def gates(e):
        tok0 = pl.multiple_of(e * 512, 512)
        xb = xs[pl.ds(tok0, 512), :].astype(BF16)
        st = lax.dot_general(rw_v[...].astype(BF16), xb, (((1,), (1,)), ((), ())),
                             preferred_element_type=F32)
        sub = _iota((16, 128), 0)
        for b in range(4):
            s = st[:, 128 * b:128 * (b + 1)]
            p = jnp.exp(s - jnp.max(s, axis=0, keepdims=True))
            p = p / jnp.sum(p, axis=0, keepdims=True)
            blk = e * 4 + b
            i0 = idx_v[pl.ds(2 * blk, 1), :]
            i1 = idx_v[pl.ds(2 * blk + 1, 1), :]
            a0 = jnp.sum(jnp.where(sub == i0, p, 0.0), axis=0, keepdims=True)
            a1 = jnp.sum(jnp.where(sub == i1, p, 0.0), axis=0, keepdims=True)
            gs = a0 + a1
            g0_v[pl.ds(blk, 1), :] = a0 / gs
            g1_v[pl.ds(blk, 1), :] = a1 / gs

    def expert(e, carry):
        row_base, sb = carry[0], carry[1:]
        nk = [misc_s[0, 4 * e + k] for k in range(NDEV)]
        n_e = nk[0] + nk[1] + nk[2] + nk[3]

        def block(bi, c):
            r4 = (row_base + bi * BM) * 4
            for j in range(4):
                lhs_b[:, 128 * j:128 * (j + 1)] = lhs_t[pl.ds(r4 + j, BM, stride=4), :].astype(BF16)
            for h in range(2):
                @pl.when(bi == 0)
                def _():
                    pltpu.make_async_copy(wv.at[0], wv.at[0], wsem.at[2 * e + h]).wait()
                y = jnp.dot(lhs_b[...], wv[2 * e + h].astype(BF16), preferred_element_type=F32)
                for jj in range(2):
                    yt[pl.ds(r4 + 2 * h + jj, BM, stride=4), :] = _pack(
                        y[:, 256 * jj:256 * jj + 128], y[:, 256 * jj + 128:256 * jj + 256])
            return c

        lax.fori_loop(0, jnp.maximum((n_e + BM - 1) // BM, 1), block, 0)

        @pl.when(e == 0)
        def _():
            pl.semaphore_wait(barrier, NDEV - 1)

        src_k = [row_base, row_base + nk[0], row_base + nk[0] + nk[1],
                 row_base + nk[0] + nk[1] + nk[2]]

        def message(m, c):
            grp = m >> 2
            dev = (me + 1 + (m & 3) * 2 + ((m & 3) >> 1)) % NDEV
            dev = jnp.where((m & 3) == 2, diag, jnp.where((m & 3) == 3, me, dev))
            n_all = misc_s[0, 4 * e + dev]
            n_a = misc_s[1, 4 * e + dev]
            src = jnp.where(dev == 0, src_k[0], jnp.where(dev == 1, src_k[1],
                            jnp.where(dev == 2, src_k[2], src_k[3])))
            dst = jnp.where(dev == 0, sb[0], jnp.where(dev == 1, sb[1],
                            jnp.where(dev == 2, sb[2], sb[3])))
            first = grp == 0
            off = jnp.where(first, 0, n_a)
            send_rows(src + off, dst + off, jnp.where(first, n_a, n_all - n_a), dev, grp)
            return c

        lax.fori_loop(0, 2 * NDEV, message, 0)
        gates(e)
        return (row_base + n_e,) + tuple(sb[k] + nk[k] for k in range(NDEV))

    carry0 = (jnp.int32(0),) + tuple(misc_s[2, k] for k in range(NDEV))
    n_local = lax.fori_loop(0, EPC, expert, carry0)[0]

    g0_cp = pltpu.make_async_copy(g0_v, g0_s, lsem.at[6])
    g1_cp = pltpu.make_async_copy(g1_v, g1_s, lsem.at[7])
    g0_cp.start()
    g1_cp.start()
    lb_cp.wait()
    gp_cp.wait()
    g0_cp.wait()
    g1_cp.wait()

    def block_rows(w, k, first=0, n=CAP):
        return gb.at[pl.ds((w * T + k * CAP + first) * 4, n * 4)]

    def remote(ref, recv, dev):
        return pltpu.make_async_remote_copy(src_ref=ref, dst_ref=ref, send_sem=p2_send,
                                            recv_sem=recv, device_id=(dev,), device_id_type=MESH)

    def combine(w):
        base = (w * T + me * CAP) * 4

        def step(pp, c):
            for u in range(8):
                p = pp * 8 + u
                word = lb_s[w, p]
                tl = word >> 20
                a0 = g0_s[w, tl]
                a1 = g1_s[w, tl]
                y0 = stg[pl.ds((word & 1023) * 4, 4), :]
                y1 = stg[pl.ds(((word >> 10) & 1023) * 4, 4), :]
                gb[pl.ds(base + p * 4, 4), :] = _pack(
                    a0 * _unpack(y0, 0) + a1 * _unpack(y1, 0),
                    a0 * _unpack(y0, 1) + a1 * _unpack(y1, 1))
            return c

        lax.fori_loop(0, CAP // 8, step, 0)

    def unpermute(w):
        def step(tt, c):
            for u in range(16):
                t = tt * 16 + u
                tmp[pl.ds(t * 4, 4), :] = gb[pl.ds(gp_s[w, t], 4), :]
            return c

        lax.fori_loop(0, T // 16, step, 0)
        rows = pl.ds(pl.multiple_of(w * T, T), T)
        for j in range(4):
            p = tmp[pl.ds(j, T, stride=4), :]
            ost[rows, 256 * j:256 * j + 128] = _unpack(p, 0)
            ost[rows, 256 * j + 128:256 * j + 256] = _unpack(p, 1)
        pltpu.make_async_copy(ost.at[rows], out_hbm.at[rows], osem).start()

    half = CAP // 2
    grp_rows = stg.at[pl.ds(0, (NW // 2) * CAP * 2 * 4)]

    def wave(i, c):
        wd = i - LA

        @pl.when((wd >= 0) & (wd < NW))
        def _():
            remote(block_rows(wd, left), dl_recv.at[wd], left).wait_recv()
            remote(block_rows(wd, left, 0, half), f_recv.at[wd], right).start()
            remote(block_rows(wd, right), dr_recv.at[wd], right).wait_recv()
            remote(block_rows(wd, right, half, half), f_recv.at[wd], left).start()

        @pl.when(i < NW)
        def _():
            @pl.when((i == 0) | (i == NW // 2))
            def _():
                pltpu.make_async_copy(grp_rows, grp_rows, p1_recv.at[i // (NW // 2)]).wait()
            combine(i)
            remote(block_rows(i, me), dl_recv.at[i], right).start()
            remote(block_rows(i, me), dr_recv.at[i], left).start()

        wu = wd - 1

        @pl.when(wu >= 0)
        def _():
            remote(block_rows(wu, diag), f_recv.at[wu], left).wait_recv()
            unpermute(wu)

        return c

    lax.fori_loop(0, NW + LA + 1, wave, 0)

    for bit in range(12, -1, -1):
        @pl.when(((n_local >> bit) & 1) == 1)
        def _():
            ref = yt.at[pl.ds(0, 4 << bit)]
            pltpu.make_async_remote_copy(src_ref=ref, dst_ref=ref, send_sem=p1_send,
                                         recv_sem=p1_recv.at[0], device_id=(me,),
                                         device_id_type=MESH).wait_send()
    sent = gb.at[pl.ds(0, NW * 3 * CAP * 4)]
    remote(sent, f_recv.at[0], me).wait_send()
    pltpu.make_async_copy(ost, out_hbm, osem).wait()


def pallas_dist_moe_top2_ep_n2048_d512_e4_h1024_kernel(
    x: jax.Array,
    router_W: jax.Array,
    route_idx: jax.Array,
    expert_W: jax.Array,
):
    idx = route_idx.astype(I32).reshape(NW, T, 2).transpose(0, 2, 1).reshape(2 * NW, T)
    rw_t = router_W.T
    vmem, smem, dma = pltpu.VMEM, pltpu.SMEM, pltpu.SemaphoreType.DMA
    scratch = [
        vmem((32, 128), I32),
        vmem((32, 128), I32),
        vmem((16, D), F32),
        vmem((N, D), F32),
        vmem((N * 4, 128), F32),
        vmem((2 * EPC, D, 512), F32),
        vmem(((RMAX + 2) * 4, 128), F32),
        vmem((BM, D), BF16),
        vmem((RMAX * 4, 128), U32),
        vmem((NW * CAP * 2 * 4, 128), U32),
        vmem((N * 4, 128), U32),
        vmem((T * 4, 128), U32),
        vmem((N, H), F32),
        vmem((32, 128), I32),
        vmem((16, 128), I32),
        vmem((16, 128), I32),
        vmem((8, 128), I32),
        vmem((16, 128), F32),
        vmem((16, 128), F32),
        smem((32, 128), I32),
        smem((16, 128), I32),
        smem((16, 128), I32),
        smem((8, 128), I32),
        smem((16, 128), F32),
        smem((16, 128), F32),
        dma((8,)),
        dma((XC,)),
        dma((2 * EPC,)),
        dma(()),
        dma(()),
        dma((2,)),
        dma(()),
        dma((NW,)),
        dma((NW,)),
        dma((NW,)),
    ]
    return pl.pallas_call(
        _body,
        out_shape=jax.ShapeDtypeStruct((N, H), F32),
        in_specs=[pl.BlockSpec(memory_space=pl.ANY)] * 4,
        out_specs=pl.BlockSpec(memory_space=pl.ANY),
        scratch_shapes=scratch,
        compiler_params=pltpu.CompilerParams(
            collective_id=0,
            vmem_limit_bytes=100 * 1024 * 1024,
            disable_bounds_checks=True,
            disable_semaphore_checks=True,
        ),
    )(x, rw_t, idx, expert_W)
```

```python
import jax
import jax.numpy as jnp
from jax import lax
from jax.experimental import pallas as pl
from jax.experimental.pallas import tpu as pltpu

I32 = jnp.int32
U32 = jnp.uint32
F32 = jnp.float32
BF16 = jnp.bfloat16
MESH = pl.DeviceIdType.MESH

N, D, H = 2048, 512, 1024
NDEV, EPC = 4, 4
NW, T, CAP = 16, 128, 32
BM = 288
BR = 32
OUT_DTYPE = BF16
XC = 8
XT = N // XC
GU = 16
LA = 3
NA = 4
UL = 2
RMAX = 2 * N + BM
TRASH = RMAX


def _iota(shape, dim):
    return lax.broadcasted_iota(I32, shape, dim)


def _cum_tot(masks, uj):
    r = masks[0].shape[0]
    h = jnp.concatenate([jnp.where(m, 1.0, 0.0).astype(BF16) for m in masks], axis=0)
    ct = jnp.dot(h, uj, preferred_element_type=F32)
    cum = [ct[r * i:r * (i + 1), 0:128] for i in range(len(masks))]
    tot = [ct[r * i:r * (i + 1), 128:256] for i in range(len(masks))]
    return cum, tot


def _shift_left_flat(x, s):
    r = x.shape[0]
    row = _iota(x.shape, 0)
    lane = _iota(x.shape, 1)
    if s < 128:
        a = pltpu.roll(x, 128 - s, 1)
        b = pltpu.roll(a, r - 1, 0)
        y = jnp.where(lane < 128 - s, a, b)
        return jnp.where((lane >= 128 - s) & (row == r - 1), 0, y)
    rs = s // 128
    y = pltpu.roll(x, r - rs, 0)
    return jnp.where(row >= r - rs, 0, y)


def _shift_left_rows(x, s):
    lane = _iota(x.shape, 1)
    return jnp.where(lane < 128 - s, pltpu.roll(x, 128 - s, 1), 0)


def _compact(word, nbits, shift):
    for s in range(nbits):
        inc = shift(word, 1 << s)
        take = ((inc >> nbits) & (inc >> s) & 1) == 1
        stay = (((word >> nbits) & 1) == 1) & (((word >> s) & 1) == 0)
        word = jnp.where(take, inc, jnp.where(stay, word, 0))
    return word


def _routing_metadata(me, idx_v, dup_v, la_v, lb_v, gp_v, misc_v):
    ui = _iota((128, 256), 0)
    ul = _iota((128, 256), 1)
    uj = jnp.where((ui < ul) | (ul >= 128), 1.0, 0.0).astype(BF16)

    e0 = idx_v[pl.ds(0, NW, stride=2), :]
    e1 = idx_v[pl.ds(1, NW, stride=2), :]
    lane = _iota((NW, T), 1)
    c0 = e0 >> 2
    c1 = e1 >> 2
    dc = (c1 - c0) & 3
    pref = jnp.where(dc == 0, c0, jnp.where(dc == 2, NDEV, jnp.where((lane & 1) == 1, c0, c1)))
    masks = [pref == k for k in range(NDEV)]
    cum, tot = _cum_tot(masks, uj)
    rank = sum(jnp.where(masks[k], cum[k], 0.0) for k in range(NDEV))
    keep = (pref < NDEV) & (rank < CAP)
    (f,), _ = _cum_tot([jnp.logical_not(keep)], uj)
    free = [CAP - jnp.minimum(tot[k], float(CAP)) for k in range(NDEV)]
    p1 = free[0]
    p2 = p1 + free[1]
    p3 = p2 + free[2]
    spill = (f >= p1).astype(I32) + (f >= p2).astype(I32) + (f >= p3).astype(I32)
    owner = jnp.where(keep, pref, spill)
    omasks = [owner == k for k in range(NDEV)]
    qcum, _ = _cum_tot(omasks, uj)
    q = sum(jnp.where(omasks[k], qcum[k], 0.0) for k in range(NDEV)).astype(I32)
    gp_v[...] = ((_iota((NW, T), 0) * T + owner * CAP + q) * 4).reshape(NW * T)

    dup_v[pl.ds(0, NW, stride=2), :] = owner
    dup_v[pl.ds(1, NW, stride=2), :] = owner
    oa = dup_v[...]
    ea = idx_v[...]
    local = (ea >> 2) == me
    cs = jnp.where(local, (ea & 3) * 4 + oa, -1)
    co = jnp.where(oa == me, ea, -1)
    cx = jnp.where(ea < EPC * me, oa, -1)
    ms = [cs == c for c in range(16)]
    mo = [co == c for c in range(16)]
    mx = [cx == k for k in range(NDEV)]
    cum_s, tot_s = _cum_tot(ms + [local], uj)
    cum_o, tot_o = _cum_tot(mo, uj)
    _, tot_x = _cum_tot(mx, uj)
    tri = jnp.where(_iota((40, 32), 1) < _iota((40, 32), 0), 1.0, 0.0).astype(BF16)
    tt = jnp.concatenate(tot_s + tot_o + tot_x, axis=1).astype(BF16)
    car = jnp.dot(tri, tt, preferred_element_type=F32)

    def blk(i):
        return car[:, 128 * i:128 * (i + 1)]

    lane1 = _iota((1, 128), 1)
    zrow = jnp.zeros((1, 128), I32)
    row_n, row_na, row_src, row_dst, row_c = zrow, zrow, zrow, zrow, zrow
    base = jnp.zeros((1, 128), F32)
    r = jnp.zeros((32, 128), F32)
    owed = [blk(33 + k)[32:33] for k in range(NDEV)]
    for c in range(16):
        cb = blk(c)
        r = r + jnp.where(ms[c], cum_s[c] + cb[0:32] + base, 0.0)
        row_n = jnp.where(lane1 == c, cb[32:33].astype(I32), row_n)
        row_na = jnp.where(lane1 == c, cb[2 * NA:2 * NA + 1].astype(I32), row_na)
        row_src = jnp.where(lane1 == c, base.astype(I32), row_src)
        row_dst = jnp.where(lane1 == c, owed[c % NDEV].astype(I32), row_dst)
        base = base + cb[32:33]
        owed[c % NDEV] = owed[c % NDEV] + cb[32:33]
    locb = blk(16)
    rl = cum_s[16] + locb[0:32]
    base = jnp.zeros((1, 128), F32)
    sg = jnp.zeros((32, 128), F32)
    for c in range(16):
        cb = blk(17 + c)
        sg = sg + jnp.where(mo[c], cum_o[c] + cb[0:32] + base, 0.0)
        base = base + cb[32:33]
    rpc = 32 // XC
    for c in range(XC):
        row_c = jnp.where(lane1 == c, locb[rpc * (c + 1):rpc * (c + 1) + 1].astype(I32), row_c)
    sub8 = _iota((8, 128), 0)
    misc = jnp.zeros((8, 128), I32)
    for i, row in enumerate((row_n, row_na, row_src, row_dst, row_c)):
        misc = jnp.where(sub8 == i, row, misc)
    misc_v[...] = misc.reshape(8 * 128)

    aidx = _iota((32, 128), 0) * 128 + _iota((32, 128), 1)
    wa = jnp.where(local, (r.astype(I32) << 13) | (1 << 12) | (aidx - rl.astype(I32)), 0)
    wa = _compact(wa, 12, _shift_left_flat)
    a = aidx + (wa & 4095)
    tok = ((a >> 8) << 7) | (a & 127)
    la_v[...] = jnp.where(((wa >> 12) & 1) == 1, (tok * 4) | (((wa >> 13) * 4) << 16),
                          (TRASH * 4) << 16).reshape(32 * 128)

    dup_v[...] = sg.astype(I32)
    s0 = dup_v[pl.ds(0, NW, stride=2), :]
    s1 = dup_v[pl.ds(1, NW, stride=2), :]
    wb = jnp.where(owner == me, (s1 << 18) | (s0 << 8) | (1 << 7) | (lane - q), 0)
    wb = _compact(wb, 7, _shift_left_rows)
    tl = lane + (wb & 127)
    lb_v[...] = jnp.where(lane < CAP,
                          ((wb >> 8) & 1023) | (((wb >> 18) & 1023) << 10) | (tl << 20),
                          0).reshape(NW * T)


def _unpack(p, i):
    bits = (p << 16) if i == 0 else (p & jnp.uint32(0xFFFF0000))
    return lax.bitcast_convert_type(bits, F32)


def _pack(lo, hi):
    lo = lax.bitcast_convert_type(lo.astype(BF16).astype(F32), U32)
    hi = lax.bitcast_convert_type(hi.astype(BF16).astype(F32), U32)
    return hi | (lo >> 16)


def _body(x_hbm, rw_hbm, idx_hbm, w_hbm, out_ref,
          idx_v, dup_v, rw_v, xs, xt, wv, lhs_t, lhs_b, acc, yt, stg, gb, tmp,
          la_v, lb_v, gp_v, misc_v, g0_v, g1_v, g0f_v, g1f_v,
          la_s, lb_s, gp_s, misc_s, g0_s, g1_s,
          lsem, xsem, wsem, p1_send, p1_recv, p2_send, dl_recv, dr_recv, f_recv):
    me = lax.axis_index("i")
    right = (me + 1) % NDEV
    left = (me + NDEV - 1) % NDEV
    diag = (me + 2) % NDEV

    idx_cp = pltpu.make_async_copy(idx_hbm, idx_v, lsem.at[0])
    rw_cp = pltpu.make_async_copy(rw_hbm, rw_v, lsem.at[1])

    def x_copy(c):
        rows = pl.ds(pl.multiple_of(c * XT, XT), XT)
        return pltpu.make_async_copy(x_hbm.at[rows], xs.at[rows], xsem.at[c])

    w_pieces = ((0, D, 0), (0, D // 2, 1), (D // 2, D // 2, 1))

    def w_copy(e, i):
        k0, nk, h = w_pieces[i]
        return pltpu.make_async_copy(w_hbm.at[e, pl.ds(k0, nk), pl.ds(512 * h, 512)],
                                     wv.at[2 * e + h, pl.ds(k0, nk), :], wsem.at[3 * e + i])

    idx_cp.start()
    for e in range(EPC):
        for i in range(3):
            w_copy(e, i).start(priority=1)
    rw_cp.start()
    barrier = pltpu.get_barrier_semaphore()
    for peer in (right, left, diag):
        pl.semaphore_signal(barrier, inc=1, device_id=(peer,), device_id_type=MESH)
    idx_cp.wait()
    for c in range(XC):
        x_copy(c).start()

    _routing_metadata(me, idx_v, dup_v, la_v, lb_v, gp_v, misc_v)
    la_cp = pltpu.make_async_copy(la_v, la_s, lsem.at[2])
    misc_cp = pltpu.make_async_copy(misc_v, misc_s, lsem.at[3])
    lb_cp = pltpu.make_async_copy(lb_v, lb_s, lsem.at[4])
    gp_cp = pltpu.make_async_copy(gp_v, gp_s, lsem.at[5])
    for cp in (misc_cp, la_cp, lb_cp, gp_cp):
        cp.start()

    def relayout(c):
        x_copy(c).wait()
        rows = pl.ds(pl.multiple_of(c * XT, XT), XT)
        for j in range(4):
            xt[pl.ds(c * (XT * 4) + j, XT, stride=4), :] = xs[rows, 128 * j:128 * (j + 1)]

    npre = 2
    for c in range(npre):
        relayout(c)
    misc_cp.wait()
    n_local = misc_s[4 * 128 + XC - 1]
    lhs_t[pl.ds(n_local * 4, BM * 4), :] = jnp.zeros((BM * 4, 128), F32)
    la_cp.wait()

    def gather_group(g, carry):
        base = g * GU
        for u in range(GU):
            w = la_s[base + u]
            lhs_t[pl.ds(w >> 16, 4), :] = xt[pl.ds(w & 0xFFFF, 4), :]
        return carry

    def x_step(c, g0):
        @pl.when(c >= npre)
        def _():
            relayout(c)
        n = misc_s[4 * 128 + c]
        g1 = jnp.where(c == XC - 1, (n + GU - 1) // GU, n // GU)
        lax.fori_loop(g0, g1, gather_group, 0)
        return g1

    lax.fori_loop(0, XC, x_step, 0)
    rw_cp.wait()

    def send_piece(src, dst, rows, dev, grp):
        pltpu.make_async_remote_copy(
            src_ref=yt.at[pl.ds(src * 4, rows * 4)],
            dst_ref=stg.at[pl.ds(dst * 4, rows * 4)],
            send_sem=p1_send, recv_sem=p1_recv.at[grp],
            device_id=(dev,), device_id_type=MESH).start()

    def send_rows(src, dst, n, dev, grp):
        def big(i, c):
            send_piece(src + i * 64, dst + i * 64, 64, dev, grp)
            return c
        lax.fori_loop(0, n >> 6, big, 0)
        for bit in range(5, -1, -1):
            @pl.when(((n >> bit) & 1) == 1)
            def _():
                off = (n >> (bit + 1)) << (bit + 1)
                send_piece(src + off, dst + off, 1 << bit, dev, grp)

    def gates(e):
        tok0 = pl.multiple_of(e * 512, 512)
        xb = xs[pl.ds(tok0, 512), :].astype(BF16)
        st = lax.dot_general(rw_v[...].astype(BF16), xb, (((1,), (1,)), ((), ())),
                             preferred_element_type=F32)
        sub = _iota((16, 128), 0)
        for b in range(4):
            s = st[:, 128 * b:128 * (b + 1)]
            p = jnp.exp(s - jnp.max(s, axis=0, keepdims=True))
            p = p / jnp.sum(p, axis=0, keepdims=True)
            blk = e * 4 + b
            i0 = idx_v[pl.ds(2 * blk, 1), :]
            i1 = idx_v[pl.ds(2 * blk + 1, 1), :]
            a0 = jnp.sum(jnp.where(sub == i0, p, 0.0), axis=0, keepdims=True)
            a1 = jnp.sum(jnp.where(sub == i1, p, 0.0), axis=0, keepdims=True)
            gs = a0 + a1
            g0_v[pl.ds(blk, 1), :] = a0 / gs
            g1_v[pl.ds(blk, 1), :] = a1 / gs

    def message(c, dev, grp):
        n_all = misc_s[c]
        n_a = misc_s[128 + c]
        off = jnp.where(grp == 0, 0, n_a)
        send_rows(misc_s[2 * 128 + c] + off, misc_s[3 * 128 + c] + off,
                  jnp.where(grp == 0, n_a, n_all - n_a), dev, grp)

    def expert(e, carry):
        row_base = misc_s[2 * 128 + 4 * e]
        n_e = misc_s[4 * e] + misc_s[4 * e + 1] + misc_s[4 * e + 2] + misc_s[4 * e + 3]

        def block(row0, rows, first):
            r4 = row0 * 4
            for j in range(4):
                lhs_b[0:rows, 128 * j:128 * (j + 1)] = (
                    lhs_t[pl.ds(r4 + j, rows, stride=4), :].astype(BF16))

            def piece(i):
                k0, nk, h = w_pieces[i]
                if first:
                    w_copy(e, i).wait()
                return jnp.dot(lhs_b[0:rows, k0:k0 + nk],
                               wv[2 * e + h, k0:k0 + nk, :].astype(BF16),
                               preferred_element_type=F32)

            def store(y, h):
                for jj in range(2):
                    yt[pl.ds(r4 + 2 * h + jj, rows, stride=4), :] = _pack(
                        y[:, 256 * jj:256 * jj + 128], y[:, 256 * jj + 128:256 * jj + 256])

            store(piece(0), 0)
            acc[0:rows, :] = piece(1)
            store(acc[0:rows, :] + piece(2), 1)

        def overflow(bi, c):
            block(row_base + BM + bi * BR, BR, False)
            return c

        block(row_base, BM, True)
        lax.fori_loop(0, (jnp.maximum(n_e - BM, 0) + BR - 1) // BR, overflow, 0)

        @pl.when(e == 0)
        def _():
            pl.semaphore_wait(barrier, NDEV - 1)

        def remote_message(m, c):
            grp = m // 3
            j = m - grp * 3
            dev = jnp.where(j == 0, diag, jnp.where(j == 1, right, left))
            message(4 * e + dev, dev, grp)
            return c

        lax.fori_loop(0, 6, remote_message, 0)
        gates(e)
        return carry

    lax.fori_loop(0, EPC, expert, 0)

    g0f_v[...] = g0_v[...].reshape(N)
    g1f_v[...] = g1_v[...].reshape(N)
    g0_cp = pltpu.make_async_copy(g0f_v, g0_s, lsem.at[6])
    g1_cp = pltpu.make_async_copy(g1f_v, g1_s, lsem.at[7])
    g0_cp.start()
    g1_cp.start()

    def own_message(m, c):
        message(4 * (m & 3) + me, me, m >> 2)
        return c

    lax.fori_loop(0, 2 * EPC, own_message, 0)
    for cp in (lb_cp, gp_cp, g0_cp, g1_cp):
        cp.wait()

    def block_rows(w, k, first=0, n=CAP):
        return gb.at[pl.ds((w * T + k * CAP + first) * 4, n * 4)]

    def remote(ref, recv, dev):
        return pltpu.make_async_remote_copy(src_ref=ref, dst_ref=ref, send_sem=p2_send,
                                            recv_sem=recv, device_id=(dev,), device_id_type=MESH)

    def combine(w):
        base = (w * T + me * CAP) * 4

        def step(pp, c):
            for u in range(8):
                p = pp * 8 + u
                word = lb_s[w * T + p]
                tl = w * T + (word >> 20)
                a0 = g0_s[tl]
                a1 = g1_s[tl]
                y0 = stg[pl.ds((word & 1023) * 4, 4), :]
                y1 = stg[pl.ds(((word >> 10) & 1023) * 4, 4), :]
                gb[pl.ds(base + p * 4, 4), :] = _pack(
                    a0 * _unpack(y0, 0) + a1 * _unpack(y1, 0),
                    a0 * _unpack(y0, 1) + a1 * _unpack(y1, 1))
            return c

        lax.fori_loop(0, CAP // 8, step, 0)

    def unpermute(w):
        def step(tt, c):
            for u in range(16):
                t = tt * 16 + u
                tmp[pl.ds(t * 4, 4), :] = gb[pl.ds(gp_s[w * T + t], 4), :]
            return c

        lax.fori_loop(0, T // 16, step, 0)
        rows = pl.ds(pl.multiple_of(w * T, T), T)
        for j in range(4):
            p = tmp[pl.ds(j, T, stride=4), :]
            out_ref[rows, 256 * j:256 * j + 128] = _unpack(p, 0).astype(OUT_DTYPE)
            out_ref[rows, 256 * j + 128:256 * j + 256] = _unpack(p, 1).astype(OUT_DTYPE)

    half = CAP // 2
    grp_rows = (stg.at[pl.ds(0, NA * CAP * 2 * 4)], stg.at[pl.ds(0, (NW - NA) * CAP * 2 * 4)])

    def wave(i, c):
        wd = i - LA

        @pl.when((wd >= 0) & (wd < NW))
        def _():
            remote(block_rows(wd, left), dl_recv.at[wd], left).wait_recv()
            remote(block_rows(wd, left, 0, half), f_recv.at[wd], right).start()
            remote(block_rows(wd, right), dr_recv.at[wd], right).wait_recv()
            remote(block_rows(wd, right, half, half), f_recv.at[wd], left).start()

        @pl.when(i < NW)
        def _():
            for g in range(2):
                @pl.when(i == g * NA)
                def _():
                    pltpu.make_async_copy(grp_rows[g], grp_rows[g], p1_recv.at[g]).wait()
            combine(i)
            remote(block_rows(i, me), dl_recv.at[i], right).start()
            remote(block_rows(i, me), dr_recv.at[i], left).start()

        @pl.when(i == NW)
        def _():
            for bit in range(12, -1, -1):
                @pl.when(((n_local >> bit) & 1) == 1)
                def _():
                    ref = yt.at[pl.ds(0, 4 << bit)]
                    pltpu.make_async_remote_copy(
                        src_ref=ref, dst_ref=ref, send_sem=p1_send, recv_sem=p1_recv.at[0],
                        device_id=(me,), device_id_type=MESH).wait_send()

        wu = wd - UL

        @pl.when(wu >= 0)
        def _():
            remote(block_rows(wu, diag), f_recv.at[wu], left).wait_recv()
            unpermute(wu)

        return c

    lax.fori_loop(0, NW + LA + UL, wave, 0)

    sent = gb.at[pl.ds(0, NW * 3 * CAP * 4)]
    remote(sent, f_recv.at[0], me).wait_send()


def pallas_dist_moe_top2_ep_n2048_d512_e4_h1024_kernel(
    x: jax.Array,
    router_W: jax.Array,
    route_idx: jax.Array,
    expert_W: jax.Array,
):
    idx = route_idx.astype(I32).reshape(NW, T, 2).transpose(0, 2, 1).reshape(2 * NW, T)
    rw_t = router_W.T
    vmem, smem, dma = pltpu.VMEM, pltpu.SMEM, pltpu.SemaphoreType.DMA
    scratch = [
        vmem((32, 128), I32),
        vmem((32, 128), I32),
        vmem((16, D), F32),
        vmem((N, D), F32),
        vmem((N * 4, 128), F32),
        vmem((2 * EPC, D, 512), F32),
        vmem(((RMAX + 2) * 4, 128), F32),
        vmem((BM, D), BF16),
        vmem((BM, 512), F32),
        vmem((RMAX * 4, 128), U32),
        vmem((NW * CAP * 2 * 4, 128), U32),
        vmem((N * 4, 128), U32),
        vmem((T * 4, 128), U32),
        vmem((2 * N,), I32),
        vmem((N,), I32),
        vmem((N,), I32),
        vmem((1024,), I32),
        vmem((16, 128), F32),
        vmem((16, 128), F32),
        vmem((N,), F32),
        vmem((N,), F32),
        smem((2 * N,), I32),
        smem((N,), I32),
        smem((N,), I32),
        smem((1024,), I32),
        smem((N,), F32),
        smem((N,), F32),
        dma((8,)),
        dma((XC,)),
        dma((3 * EPC,)),
        dma(()),
        dma((2,)),
        dma(()),
        dma((NW,)),
        dma((NW,)),
        dma((NW,)),
    ]
    return pl.pallas_call(
        _body,
        out_shape=jax.ShapeDtypeStruct((N, H), OUT_DTYPE),
        in_specs=[pl.BlockSpec(memory_space=pl.ANY)] * 4,
        out_specs=pl.BlockSpec(memory_space=pltpu.VMEM),
        scratch_shapes=scratch,
        compiler_params=pltpu.CompilerParams(
            collective_id=0,
            vmem_limit_bytes=64 * 1024 * 1024,
            disable_bounds_checks=True,
            disable_semaphore_checks=True,
        ),
    )(x, rw_t, idx, expert_W)
```

```python
import jax
import jax.numpy as jnp
from jax import lax
from jax.experimental import pallas as pl
from jax.experimental.pallas import tpu as pltpu

I32 = jnp.int32
U32 = jnp.uint32
F32 = jnp.float32
BF16 = jnp.bfloat16
MESH = pl.DeviceIdType.MESH

N, D, H = 2048, 512, 1024
NDEV, EPC = 4, 4
NW, T, CAP = 16, 128, 32
BM = 288
BR = 32
OUT_DTYPE = BF16
XC = 8
XT = N // XC
GU = 16
LA = 3
NA = 4
UL = 2
RMAX = 2 * N + BM
TRASH = RMAX


def _iota(shape, dim):
    return lax.broadcasted_iota(I32, shape, dim)


def _cum_tot(masks, uj):
    r = masks[0].shape[0]
    h = jnp.concatenate([jnp.where(m, 1.0, 0.0).astype(BF16) for m in masks], axis=0)
    ct = jnp.dot(h, uj, preferred_element_type=F32)
    cum = [ct[r * i:r * (i + 1), 0:128] for i in range(len(masks))]
    tot = [ct[r * i:r * (i + 1), 128:256] for i in range(len(masks))]
    return cum, tot


def _shift_left_flat(x, s):
    r = x.shape[0]
    row = _iota(x.shape, 0)
    lane = _iota(x.shape, 1)
    if s < 128:
        a = pltpu.roll(x, 128 - s, 1)
        b = pltpu.roll(a, r - 1, 0)
        y = jnp.where(lane < 128 - s, a, b)
        return jnp.where((lane >= 128 - s) & (row == r - 1), 0, y)
    rs = s // 128
    y = pltpu.roll(x, r - rs, 0)
    return jnp.where(row >= r - rs, 0, y)


def _shift_left_rows(x, s):
    lane = _iota(x.shape, 1)
    return jnp.where(lane < 128 - s, pltpu.roll(x, 128 - s, 1), 0)


def _compact(word, nbits, shift):
    for s in range(nbits):
        inc = shift(word, 1 << s)
        take = ((inc >> nbits) & (inc >> s) & 1) == 1
        stay = (((word >> nbits) & 1) == 1) & (((word >> s) & 1) == 0)
        word = jnp.where(take, inc, jnp.where(stay, word, 0))
    return word


def _routing_metadata(me, idx_v, dup_v, la_v, lb_v, gp_v, misc_v):
    ui = _iota((128, 256), 0)
    ul = _iota((128, 256), 1)
    uj = jnp.where((ui < ul) | (ul >= 128), 1.0, 0.0).astype(BF16)

    e0 = idx_v[pl.ds(0, NW, stride=2), :]
    e1 = idx_v[pl.ds(1, NW, stride=2), :]
    lane = _iota((NW, T), 1)
    c0 = e0 >> 2
    c1 = e1 >> 2
    dc = (c1 - c0) & 3
    same = dc == 0
    adj = (dc & 1) == 1
    low = jnp.where(dc == 1, c0, c1)
    high = jnp.where(dc == 1, c1, c0)
    kinds = ([same & (c0 == k) for k in range(NDEV)] + [adj & (low == k) for k in range(NDEV)]
             + [(dc == 2) & ((c0 & 1) == k) for k in range(2)])
    kcum, ktot = _cum_tot(kinds, uj)
    ns, npair, f02, f13 = ktot[0:4], ktot[4:8], ktot[8], ktot[9]
    cap = float(CAP)
    c_r0 = npair[0]
    c_r1 = npair[0] + npair[1] + ns[1] + f13 - cap
    c_r2 = 2 * cap - ns[0] - ns[3] - npair[3]
    c_r3 = cap - ns[0]
    c_l0 = ns[0] + npair[3] - cap + f02
    c_l2 = cap - ns[1] - npair[0]
    c_l3 = 2 * cap - ns[1] - ns[2] - npair[0] - npair[1]
    g_x = c_l0 + c_l2 + c_l3 - c_r0 - c_r1 - c_r2 - c_r3
    g_a = c_r0 + c_r1 - c_l3 - c_l0
    g_b = c_l0 - c_r1 - c_r2

    def quota(v, most):
        return jnp.clip(jnp.floor(v + 0.5), 0.0, most)

    x0 = quota((-12 * g_x - 8 * g_a + 8 * g_b) / 32, npair[0])
    qa = quota((-8 * g_x - 16 * g_a) / 32, f02)
    qb = quota((8 * g_x - 16 * g_b) / 32, f13)
    x1 = quota(cap - ns[1] - npair[0] + x0 - qa, npair[1])
    x2 = quota(cap - ns[2] - npair[1] + x1 - f13 + qb, npair[2])
    x3 = quota(cap - ns[3] - npair[2] + x2 - f02 + qa, npair[3])
    to_low = ((kinds[4] & (kcum[4] < x0)) | (kinds[5] & (kcum[5] < x1))
              | (kinds[6] & (kcum[6] < x2)) | (kinds[7] & (kcum[7] < x3)))
    pref = jnp.where(same, c0, jnp.where(
        adj, jnp.where(to_low, low, high),
        jnp.where(kinds[8], jnp.where(kcum[8] < qa, 1, 3), jnp.where(kcum[9] < qb, 0, 2))))
    masks = [pref == k for k in range(NDEV)]
    cum, tot = _cum_tot(masks, uj)
    rank = sum(jnp.where(masks[k], cum[k], 0.0) for k in range(NDEV))
    keep = rank < CAP
    (f,), _ = _cum_tot([jnp.logical_not(keep)], uj)
    free = [CAP - jnp.minimum(tot[k], float(CAP)) for k in range(NDEV)]
    p1 = free[0]
    p2 = p1 + free[1]
    p3 = p2 + free[2]
    spill = (f >= p1).astype(I32) + (f >= p2).astype(I32) + (f >= p3).astype(I32)
    owner = jnp.where(keep, pref, spill)
    omasks = [owner == k for k in range(NDEV)]
    qcum, _ = _cum_tot(omasks, uj)
    q = sum(jnp.where(omasks[k], qcum[k], 0.0) for k in range(NDEV)).astype(I32)
    gp_v[...] = ((_iota((NW, T), 0) * T + owner * CAP + q) * 4).reshape(NW * T)

    dup_v[pl.ds(0, NW, stride=2), :] = owner
    dup_v[pl.ds(1, NW, stride=2), :] = owner
    oa = dup_v[...]
    ea = idx_v[...]
    local = (ea >> 2) == me
    cs = jnp.where(local, (ea & 3) * 4 + oa, -1)
    co = jnp.where(oa == me, ea, -1)
    cx = jnp.where(ea < EPC * me, oa, -1)
    ms = [cs == c for c in range(16)]
    mo = [co == c for c in range(16)]
    mx = [cx == k for k in range(NDEV)]
    cum_s, tot_s = _cum_tot(ms + [local], uj)
    cum_o, tot_o = _cum_tot(mo, uj)
    _, tot_x = _cum_tot(mx, uj)
    tri = jnp.where(_iota((40, 32), 1) < _iota((40, 32), 0), 1.0, 0.0).astype(BF16)
    tt = jnp.concatenate(tot_s + tot_o + tot_x, axis=1).astype(BF16)
    car = jnp.dot(tri, tt, preferred_element_type=F32)

    def blk(i):
        return car[:, 128 * i:128 * (i + 1)]

    lane1 = _iota((1, 128), 1)
    zrow = jnp.zeros((1, 128), I32)
    row_n, row_na, row_src, row_dst, row_c = zrow, zrow, zrow, zrow, zrow
    base = jnp.zeros((1, 128), F32)
    r = jnp.zeros((32, 128), F32)
    owed = [blk(33 + k)[32:33] for k in range(NDEV)]
    for c in range(16):
        cb = blk(c)
        r = r + jnp.where(ms[c], cum_s[c] + cb[0:32] + base, 0.0)
        row_n = jnp.where(lane1 == c, cb[32:33].astype(I32), row_n)
        row_na = jnp.where(lane1 == c, cb[2 * NA:2 * NA + 1].astype(I32), row_na)
        row_src = jnp.where(lane1 == c, base.astype(I32), row_src)
        row_dst = jnp.where(lane1 == c, owed[c % NDEV].astype(I32), row_dst)
        base = base + cb[32:33]
        owed[c % NDEV] = owed[c % NDEV] + cb[32:33]
    locb = blk(16)
    rl = cum_s[16] + locb[0:32]
    base = jnp.zeros((1, 128), F32)
    sg = jnp.zeros((32, 128), F32)
    for c in range(16):
        cb = blk(17 + c)
        sg = sg + jnp.where(mo[c], cum_o[c] + cb[0:32] + base, 0.0)
        base = base + cb[32:33]
    rpc = 32 // XC
    for c in range(XC):
        row_c = jnp.where(lane1 == c, locb[rpc * (c + 1):rpc * (c + 1) + 1].astype(I32), row_c)
    sub8 = _iota((8, 128), 0)
    misc = jnp.zeros((8, 128), I32)
    for i, row in enumerate((row_n, row_na, row_src, row_dst, row_c)):
        misc = jnp.where(sub8 == i, row, misc)
    misc_v[...] = misc.reshape(8 * 128)

    aidx = _iota((32, 128), 0) * 128 + _iota((32, 128), 1)
    wa = jnp.where(local, (r.astype(I32) << 13) | (1 << 12) | (aidx - rl.astype(I32)), 0)
    wa = _compact(wa, 12, _shift_left_flat)
    a = aidx + (wa & 4095)
    tok = ((a >> 8) << 7) | (a & 127)
    la_v[...] = jnp.where(((wa >> 12) & 1) == 1, (tok * 4) | (((wa >> 13) * 4) << 16),
                          (TRASH * 4) << 16).reshape(32 * 128)

    dup_v[...] = sg.astype(I32)
    s0 = dup_v[pl.ds(0, NW, stride=2), :]
    s1 = dup_v[pl.ds(1, NW, stride=2), :]
    wb = jnp.where(owner == me, (s1 << 18) | (s0 << 8) | (1 << 7) | (lane - q), 0)
    wb = _compact(wb, 7, _shift_left_rows)
    tl = lane + (wb & 127)
    lb_v[...] = jnp.where(lane < CAP,
                          ((wb >> 8) & 1023) | (((wb >> 18) & 1023) << 10) | (tl << 20),
                          0).reshape(NW * T)


def _unpack(p, i):
    bits = (p << 16) if i == 0 else (p & jnp.uint32(0xFFFF0000))
    return lax.bitcast_convert_type(bits, F32)


def _pack(lo, hi):
    lo = lax.bitcast_convert_type(lo.astype(BF16).astype(F32), U32)
    hi = lax.bitcast_convert_type(hi.astype(BF16).astype(F32), U32)
    return hi | (lo >> 16)


def _body(x_hbm, rw_hbm, idx_hbm, w_hbm, out_ref,
          idx_v, dup_v, rw_v, xs, xt, wv, lhs_t, lhs_b, acc, yt, stg, gb, tmp,
          la_v, lb_v, gp_v, misc_v, g0_v, g1_v, g0f_v, g1f_v,
          la_s, lb_s, gp_s, misc_s, g0_s, g1_s,
          lsem, xsem, wsem, p1_send, p1_recv, p2_send, dl_recv, dr_recv, f_recv):
    me = lax.axis_index("i")
    right = (me + 1) % NDEV
    left = (me + NDEV - 1) % NDEV
    diag = (me + 2) % NDEV

    idx_cp = pltpu.make_async_copy(idx_hbm, idx_v, lsem.at[0])
    rw_cp = pltpu.make_async_copy(rw_hbm, rw_v, lsem.at[1])

    def x_copy(c):
        rows = pl.ds(pl.multiple_of(c * XT, XT), XT)
        return pltpu.make_async_copy(x_hbm.at[rows], xs.at[rows], xsem.at[c])

    w_pieces = ((0, D, 0), (0, D // 2, 1), (D // 2, D // 2, 1))

    def w_copy(e, i):
        k0, nk, h = w_pieces[i]
        return pltpu.make_async_copy(w_hbm.at[e, pl.ds(k0, nk), pl.ds(512 * h, 512)],
                                     wv.at[2 * e + h, pl.ds(k0, nk), :], wsem.at[3 * e + i])

    idx_cp.start()
    for e in range(EPC):
        for i in range(3):
            w_copy(e, i).start(priority=1)
    rw_cp.start()
    barrier = pltpu.get_barrier_semaphore()
    for peer in (right, left, diag):
        pl.semaphore_signal(barrier, inc=1, device_id=(peer,), device_id_type=MESH)
    idx_cp.wait()
    for c in range(XC):
        x_copy(c).start()

    _routing_metadata(me, idx_v, dup_v, la_v, lb_v, gp_v, misc_v)
    la_cp = pltpu.make_async_copy(la_v, la_s, lsem.at[2])
    misc_cp = pltpu.make_async_copy(misc_v, misc_s, lsem.at[3])
    lb_cp = pltpu.make_async_copy(lb_v, lb_s, lsem.at[4])
    gp_cp = pltpu.make_async_copy(gp_v, gp_s, lsem.at[5])
    for cp in (misc_cp, la_cp, lb_cp, gp_cp):
        cp.start()

    def relayout(c):
        x_copy(c).wait()
        rows = pl.ds(pl.multiple_of(c * XT, XT), XT)
        for j in range(4):
            xt[pl.ds(c * (XT * 4) + j, XT, stride=4), :] = xs[rows, 128 * j:128 * (j + 1)]

    npre = 2
    for c in range(npre):
        relayout(c)
    misc_cp.wait()
    n_local = misc_s[4 * 128 + XC - 1]
    lhs_t[pl.ds(n_local * 4, BM * 4), :] = jnp.zeros((BM * 4, 128), F32)
    la_cp.wait()

    def gather_group(g, carry):
        base = g * GU
        for u in range(GU):
            w = la_s[base + u]
            lhs_t[pl.ds(w >> 16, 4), :] = xt[pl.ds(w & 0xFFFF, 4), :]
        return carry

    def x_step(c, g0):
        @pl.when(c >= npre)
        def _():
            relayout(c)
        n = misc_s[4 * 128 + c]
        g1 = jnp.where(c == XC - 1, (n + GU - 1) // GU, n // GU)
        lax.fori_loop(g0, g1, gather_group, 0)
        return g1

    lax.fori_loop(0, XC, x_step, 0)
    rw_cp.wait()

    def send_piece(src, dst, rows, dev, grp):
        pltpu.make_async_remote_copy(
            src_ref=yt.at[pl.ds(src * 4, rows * 4)],
            dst_ref=stg.at[pl.ds(dst * 4, rows * 4)],
            send_sem=p1_send, recv_sem=p1_recv.at[grp],
            device_id=(dev,), device_id_type=MESH).start()

    def send_rows(src, dst, n, dev, grp):
        def big(i, c):
            send_piece(src + i * 64, dst + i * 64, 64, dev, grp)
            return c
        lax.fori_loop(0, n >> 6, big, 0)
        for bit in range(5, -1, -1):
            @pl.when(((n >> bit) & 1) == 1)
            def _():
                off = (n >> (bit + 1)) << (bit + 1)
                send_piece(src + off, dst + off, 1 << bit, dev, grp)

    def gates(e):
        tok0 = pl.multiple_of(e * 512, 512)
        xb = xs[pl.ds(tok0, 512), :].astype(BF16)
        st = lax.dot_general(rw_v[...].astype(BF16), xb, (((1,), (1,)), ((), ())),
                             preferred_element_type=F32)
        sub = _iota((16, 128), 0)
        for b in range(4):
            s = st[:, 128 * b:128 * (b + 1)]
            p = jnp.exp(s - jnp.max(s, axis=0, keepdims=True))
            p = p / jnp.sum(p, axis=0, keepdims=True)
            blk = e * 4 + b
            i0 = idx_v[pl.ds(2 * blk, 1), :]
            i1 = idx_v[pl.ds(2 * blk + 1, 1), :]
            a0 = jnp.sum(jnp.where(sub == i0, p, 0.0), axis=0, keepdims=True)
            a1 = jnp.sum(jnp.where(sub == i1, p, 0.0), axis=0, keepdims=True)
            gs = a0 + a1
            g0_v[pl.ds(blk, 1), :] = a0 / gs
            g1_v[pl.ds(blk, 1), :] = a1 / gs

    def message(c, dev, grp):
        n_a = misc_s[128 + c]
        n = jnp.where(grp == 0, n_a, misc_s[c] - n_a)

        @pl.when(n > 0)
        def _():
            off = jnp.where(grp == 0, 0, n_a)
            send_rows(misc_s[2 * 128 + c] + off, misc_s[3 * 128 + c] + off, n, dev, grp)

    def expert(e, carry):
        row_base = misc_s[2 * 128 + 4 * e]
        n_e = misc_s[4 * e] + misc_s[4 * e + 1] + misc_s[4 * e + 2] + misc_s[4 * e + 3]

        def block(row0, rows, first):
            r4 = row0 * 4
            for j in range(4):
                lhs_b[0:rows, 128 * j:128 * (j + 1)] = (
                    lhs_t[pl.ds(r4 + j, rows, stride=4), :].astype(BF16))

            def piece(i):
                k0, nk, h = w_pieces[i]
                if first:
                    w_copy(e, i).wait()
                return jnp.dot(lhs_b[0:rows, k0:k0 + nk],
                               wv[2 * e + h, k0:k0 + nk, :].astype(BF16),
                               preferred_element_type=F32)

            def store(y, h):
                for jj in range(2):
                    yt[pl.ds(r4 + 2 * h + jj, rows, stride=4), :] = _pack(
                        y[:, 256 * jj:256 * jj + 128], y[:, 256 * jj + 128:256 * jj + 256])

            store(piece(0), 0)
            acc[0:rows, :] = piece(1)
            store(acc[0:rows, :] + piece(2), 1)

        def overflow(bi, c):
            block(row_base + BM + bi * BR, BR, False)
            return c

        block(row_base, BM, True)
        lax.fori_loop(0, (jnp.maximum(n_e - BM, 0) + BR - 1) // BR, overflow, 0)

        @pl.when(e == 0)
        def _():
            pl.semaphore_wait(barrier, NDEV - 1)

        def remote_message(m, c):
            grp = m // 3
            j = m - grp * 3
            dev = jnp.where(j == 0, diag, jnp.where(j == 1, right, left))
            message(4 * e + dev, dev, grp)
            return c

        lax.fori_loop(0, 6, remote_message, 0)
        gates(e)
        return carry

    lax.fori_loop(0, EPC, expert, 0)

    g0f_v[...] = g0_v[...].reshape(N)
    g1f_v[...] = g1_v[...].reshape(N)
    g0_cp = pltpu.make_async_copy(g0f_v, g0_s, lsem.at[6])
    g1_cp = pltpu.make_async_copy(g1f_v, g1_s, lsem.at[7])
    g0_cp.start()
    g1_cp.start()

    def own_message(m, c):
        message(4 * (m & 3) + me, me, m >> 2)
        return c

    lax.fori_loop(0, 2 * EPC, own_message, 0)
    for cp in (lb_cp, gp_cp, g0_cp, g1_cp):
        cp.wait()

    def block_rows(w, k, first=0, n=CAP):
        return gb.at[pl.ds((w * T + k * CAP + first) * 4, n * 4)]

    def remote(ref, recv, dev):
        return pltpu.make_async_remote_copy(src_ref=ref, dst_ref=ref, send_sem=p2_send,
                                            recv_sem=recv, device_id=(dev,), device_id_type=MESH)

    def combine(w):
        base = (w * T + me * CAP) * 4

        def step(pp, c):
            for u in range(8):
                p = pp * 8 + u
                word = lb_s[w * T + p]
                tl = w * T + (word >> 20)
                a0 = g0_s[tl]
                a1 = g1_s[tl]
                y0 = stg[pl.ds((word & 1023) * 4, 4), :]
                y1 = stg[pl.ds(((word >> 10) & 1023) * 4, 4), :]
                gb[pl.ds(base + p * 4, 4), :] = _pack(
                    a0 * _unpack(y0, 0) + a1 * _unpack(y1, 0),
                    a0 * _unpack(y0, 1) + a1 * _unpack(y1, 1))
            return c

        lax.fori_loop(0, CAP // 8, step, 0)

    def unpermute(w):
        def step(tt, c):
            for u in range(16):
                t = tt * 16 + u
                tmp[pl.ds(t * 4, 4), :] = gb[pl.ds(gp_s[w * T + t], 4), :]
            return c

        lax.fori_loop(0, T // 16, step, 0)
        rows = pl.ds(pl.multiple_of(w * T, T), T)
        for j in range(4):
            p = tmp[pl.ds(j, T, stride=4), :]
            out_ref[rows, 256 * j:256 * j + 128] = _unpack(p, 0).astype(OUT_DTYPE)
            out_ref[rows, 256 * j + 128:256 * j + 256] = _unpack(p, 1).astype(OUT_DTYPE)

    half = CAP // 2
    grp_rows = (stg.at[pl.ds(0, NA * CAP * 2 * 4)], stg.at[pl.ds(0, (NW - NA) * CAP * 2 * 4)])

    def wave(i, c):
        wd = i - LA

        @pl.when((wd >= 0) & (wd < NW))
        def _():
            remote(block_rows(wd, left), dl_recv.at[wd], left).wait_recv()
            remote(block_rows(wd, left, 0, half), f_recv.at[wd], right).start()
            remote(block_rows(wd, right), dr_recv.at[wd], right).wait_recv()
            remote(block_rows(wd, right, half, half), f_recv.at[wd], left).start()

        @pl.when(i < NW)
        def _():
            for g in range(2):
                @pl.when(i == g * NA)
                def _():
                    pltpu.make_async_copy(grp_rows[g], grp_rows[g], p1_recv.at[g]).wait()
            combine(i)
            remote(block_rows(i, me), dl_recv.at[i], right).start()
            remote(block_rows(i, me), dr_recv.at[i], left).start()

        @pl.when(i == NW)
        def _():
            for bit in range(12, -1, -1):
                @pl.when(((n_local >> bit) & 1) == 1)
                def _():
                    ref = yt.at[pl.ds(0, 4 << bit)]
                    pltpu.make_async_remote_copy(
                        src_ref=ref, dst_ref=ref, send_sem=p1_send, recv_sem=p1_recv.at[0],
                        device_id=(me,), device_id_type=MESH).wait_send()

        wu = wd - UL

        @pl.when(wu >= 0)
        def _():
            remote(block_rows(wu, diag), f_recv.at[wu], left).wait_recv()
            unpermute(wu)

        return c

    lax.fori_loop(0, NW + LA + UL, wave, 0)

    sent = gb.at[pl.ds(0, NW * 3 * CAP * 4)]
    remote(sent, f_recv.at[0], me).wait_send()


def pallas_dist_moe_top2_ep_n2048_d512_e4_h1024_kernel(
    x: jax.Array,
    router_W: jax.Array,
    route_idx: jax.Array,
    expert_W: jax.Array,
):
    idx = route_idx.astype(I32).reshape(NW, T, 2).transpose(0, 2, 1).reshape(2 * NW, T)
    rw_t = router_W.T
    vmem, smem, dma = pltpu.VMEM, pltpu.SMEM, pltpu.SemaphoreType.DMA
    scratch = [
        vmem((32, 128), I32),
        vmem((32, 128), I32),
        vmem((16, D), F32),
        vmem((N, D), F32),
        vmem((N * 4, 128), F32),
        vmem((2 * EPC, D, 512), F32),
        vmem(((RMAX + 2) * 4, 128), F32),
        vmem((BM, D), BF16),
        vmem((BM, 512), F32),
        vmem((RMAX * 4, 128), U32),
        vmem((NW * CAP * 2 * 4, 128), U32),
        vmem((N * 4, 128), U32),
        vmem((T * 4, 128), U32),
        vmem((2 * N,), I32),
        vmem((N,), I32),
        vmem((N,), I32),
        vmem((1024,), I32),
        vmem((16, 128), F32),
        vmem((16, 128), F32),
        vmem((N,), F32),
        vmem((N,), F32),
        smem((2 * N,), I32),
        smem((N,), I32),
        smem((N,), I32),
        smem((1024,), I32),
        smem((N,), F32),
        smem((N,), F32),
        dma((8,)),
        dma((XC,)),
        dma((3 * EPC,)),
        dma(()),
        dma((2,)),
        dma(()),
        dma((NW,)),
        dma((NW,)),
        dma((NW,)),
    ]
    return pl.pallas_call(
        _body,
        out_shape=jax.ShapeDtypeStruct((N, H), OUT_DTYPE),
        in_specs=[pl.BlockSpec(memory_space=pl.ANY)] * 4,
        out_specs=pl.BlockSpec(memory_space=pltpu.VMEM),
        scratch_shapes=scratch,
        compiler_params=pltpu.CompilerParams(
            collective_id=0,
            vmem_limit_bytes=64 * 1024 * 1024,
            disable_bounds_checks=True,
            disable_semaphore_checks=True,
        ),
    )(x, rw_t, idx, expert_W)
```
